```python
import numpy as np

kernel_name = "dist_rope_attn_qseq_b2_sq128_d512_hq4_dh64"

def setup_inputs():
    x = np.random.randn(2, 512, 512).astype(np.float32)
    Wq = np.random.randn(512, 256).astype(np.float32) * 0.02
    Wk = np.random.randn(512, 256).astype(np.float32) * 0.02
    Wv = np.random.randn(512, 256).astype(np.float32) * 0.02
    Wo = np.random.randn(256, 512).astype(np.float32) * 0.02
    return {"x": x, "Wq": Wq, "Wk": Wk, "Wv": Wv, "Wo": Wo}

def reference(x, Wq, Wk, Wv, Wo):
    B, Sq, Hq, Dh = 2, 512, 4, 64
    inv = 1.0 / (10000.0 ** (np.arange(0, Dh, 2) / Dh))
    pos = np.arange(Sq)[:, None] * inv[None, :]
    cos = np.repeat(np.cos(pos), 2, axis=-1).astype(np.float32)
    sin = np.repeat(np.sin(pos), 2, axis=-1).astype(np.float32)
    def rot(t):
        t2 = t.reshape(B, Sq, Hq, Dh // 2, 2)
        t_r = np.stack([-t2[..., 1], t2[..., 0]], axis=-1).reshape(B, Sq, Hq, Dh)
        return t * cos[None, :, None, :] + t_r * sin[None, :, None, :]
    Q = rot((x @ Wq).reshape(B, Sq, Hq, Dh))
    K = rot((x @ Wk).reshape(B, Sq, Hq, Dh))
    V = (x @ Wv).reshape(B, Sq, Hq, Dh)
    s = np.einsum('bihd,bjhd->bhij', Q, K).astype(np.float32) * 0.125
    s_max = s.max(axis=-1, keepdims=True)
    w = np.exp(s - s_max)
    w = w / w.sum(axis=-1, keepdims=True)
    ctx = np.einsum('bhij,bjhd->bihd', w, V).reshape(B, Sq, Hq * Dh)
    return ctx @ Wo
```

```python
import math

import jax
import jax.numpy as jnp
from jax import lax
from jax.experimental import pallas as pl
from jax.experimental.pallas import tpu as pltpu

N_DEV = 4
B = 2
SQ = 128
D = 512
HQ = 4
DH = 64
HD = HQ * DH
ROWS = B * SQ


def pallas_dist_rope_attn_qseq_b2_sq128_d512_hq4_dh64_kernel(
    x: jax.Array,
    Wq: jax.Array,
    Wk: jax.Array,
    Wv: jax.Array,
    Wo: jax.Array,
):
    bf16 = jnp.bfloat16
    f32 = jnp.float32

    def body(x_ref, wq_ref, wk_ref, wv_ref, wo_ref, out_ref,
             kv_ref, ctx_ref, send_sems, recv_sems):
        my = lax.axis_index("i")

        row = lax.broadcasted_iota(jnp.int32, (ROWS, HD), 0)
        lane = lax.broadcasted_iota(jnp.int32, (ROWS, HD), 1)
        pos = (row % SQ + my * SQ).astype(f32)
        dd = lane % DH
        even = (lane % 2) == 0
        fi = (dd - (dd % 2)).astype(f32)
        inv = jnp.exp(fi * (-math.log(10000.0) / DH))
        ang = pos * inv
        cos = jnp.cos(ang)
        sin = jnp.sin(ang)

        def rope(t):
            t_next = pltpu.roll(t, HD - 1, 1)
            t_prev = pltpu.roll(t, 1, 1)
            t_r = jnp.where(even, -t_next, t_prev)
            return t * cos + t_r * sin

        xb = x_ref[...].astype(bf16)

        k = jnp.dot(xb, wk_ref[...].astype(bf16), preferred_element_type=f32)
        v = jnp.dot(xb, wv_ref[...].astype(bf16), preferred_element_type=f32)
        k = rope(k)
        kv_ref[my, :, 0:HD] = k.astype(bf16)
        kv_ref[my, :, HD:2 * HD] = v.astype(bf16)

        copies = []
        for o in range(1, N_DEV):
            dst = (my + o) % N_DEV
            c = pltpu.make_async_remote_copy(
                src_ref=kv_ref.at[my],
                dst_ref=kv_ref.at[my],
                send_sem=send_sems.at[o - 1],
                recv_sem=recv_sems.at[o - 1],
                device_id=(dst,),
                device_id_type=pl.DeviceIdType.MESH,
            )
            c.start()
            copies.append(c)

        q = jnp.dot(xb, wq_ref[...].astype(bf16), preferred_element_type=f32)
        q = (rope(q) * 0.125).astype(bf16)

        for c in copies:
            c.wait_send()
        for o in range(1, N_DEV):
            src = (my - o) % N_DEV
            r = pltpu.make_async_remote_copy(
                src_ref=kv_ref.at[src],
                dst_ref=kv_ref.at[src],
                send_sem=send_sems.at[o - 1],
                recv_sem=recv_sems.at[o - 1],
                device_id=(src,),
                device_id_type=pl.DeviceIdType.MESH,
            )
            r.wait_recv()

        for b in range(B):
            for h in range(HQ):
                qbh = q[b * SQ:(b + 1) * SQ, h * DH:(h + 1) * DH]
                kbh = kv_ref[:, b * SQ:(b + 1) * SQ, h * DH:(h + 1) * DH]
                kbh = kbh.reshape(N_DEV * SQ, DH)
                vbh = kv_ref[:, b * SQ:(b + 1) * SQ, HD + h * DH:HD + (h + 1) * DH]
                vbh = vbh.reshape(N_DEV * SQ, DH)
                s = lax.dot_general(qbh, kbh, (((1,), (1,)), ((), ())),
                                    preferred_element_type=f32)
                m = jnp.max(s, axis=-1, keepdims=True)
                p = jnp.exp(s - m)
                l = jnp.sum(p, axis=-1, keepdims=True)
                ctx = jnp.dot(p.astype(bf16), vbh, preferred_element_type=f32)
                ctx = ctx / l
                ctx_ref[b * SQ:(b + 1) * SQ, h * DH:(h + 1) * DH] = ctx

        out_ref[...] = jnp.dot(ctx_ref[...].astype(bf16), wo_ref[...].astype(bf16),
                               preferred_element_type=f32)

    out = pl.pallas_call(
        body,
        out_shape=jax.ShapeDtypeStruct((ROWS, D), f32),
        in_specs=[pl.BlockSpec(memory_space=pltpu.VMEM)] * 5,
        out_specs=pl.BlockSpec(memory_space=pltpu.VMEM),
        scratch_shapes=[
            pltpu.VMEM((N_DEV, ROWS, 2 * HD), bf16),
            pltpu.VMEM((ROWS, HD), f32),
            pltpu.SemaphoreType.DMA((N_DEV - 1,)),
            pltpu.SemaphoreType.DMA((N_DEV - 1,)),
        ],
    )(x.reshape(ROWS, D), Wq, Wk, Wv, Wo)
    return out.reshape(B, SQ, D)
```

```python
import math

import jax
import jax.numpy as jnp
from jax import lax
from jax.experimental import pallas as pl
from jax.experimental.pallas import tpu as pltpu

N_DEV = 4
B = 2
SQ = 128
D = 512
HQ = 4
DH = 64
HD = HQ * DH
LANES = 128
HALF = SQ // 2


def pallas_dist_rope_attn_qseq_b2_sq128_d512_hq4_dh64_kernel(
    x: jax.Array,
    Wq: jax.Array,
    Wk: jax.Array,
    Wv: jax.Array,
    Wo: jax.Array,
):
    bf16 = jnp.bfloat16
    f32 = jnp.float32

    def body(x_hbm, wq_hbm, wk_hbm, wv_hbm, wo_hbm, out_ref,
             xin, wqf, wkf, wvf, wof,
             A, RX, KVO, KVC, RKV, wkv16, wq16, wo16,
             qt_ref, m_ref, l_ref, acc_ref,
             lsem, ssem, rsem):
        my = lax.axis_index("i")
        left = (my + N_DEV - 1) % N_DEV
        right = (my + 1) % N_DEV

        pieces = [(0, 0), (1, 0), (0, 1), (1, 1)]
        cxs = []
        for n, (b, hf) in enumerate(pieces):
            c = pltpu.make_async_copy(x_hbm.at[b, pl.ds(hf * HALF, HALF)],
                                      xin.at[b, pl.ds(hf * HALF, HALF)], lsem.at[n])
            c.start()
            cxs.append(c)

        bsem = pltpu.get_barrier_semaphore()
        for nb in (left, right):
            pl.semaphore_signal(bsem, inc=1, device_id=(nb,),
                                device_id_type=pl.DeviceIdType.MESH)

        cwk = pltpu.make_async_copy(wk_hbm, wkf, lsem.at[4])
        cwv = pltpu.make_async_copy(wv_hbm, wvf, lsem.at[5])
        cwk.start()
        cwv.start()

        def rdma(src, dst, dev, i):
            return pltpu.make_async_remote_copy(
                src_ref=src, dst_ref=dst,
                send_sem=ssem.at[i], recv_sem=rsem.at[i],
                device_id=(dev,), device_id_type=pl.DeviceIdType.MESH)

        cwq = pltpu.make_async_copy(wq_hbm, wqf, lsem.at[6])
        cwo = pltpu.make_async_copy(wo_hbm, wof, lsem.at[7])

        sends = []
        for n, (b, hf) in enumerate(pieces):
            rows = pl.ds(hf * HALF, HALF)
            cxs[n].wait()
            A[b, rows] = xin[b, rows].astype(bf16)
            if n == 0:
                pl.semaphore_wait(bsem, 2)
            s = rdma(A.at[b, rows], RX.at[b, rows], right if b == 0 else left, n)
            s.start()
            sends.append(s)
        cwq.start()
        cwo.start()

        def theta_of(shape):
            ln = lax.broadcasted_iota(jnp.int32, shape, 1) % DH
            fi = (ln - (ln % 2)).astype(f32)
            return jnp.exp(fi * (-math.log(10000.0) / DH))

        ang_a = lax.broadcasted_iota(jnp.int32, (8, LANES), 0).astype(f32) * theta_of((8, LANES))
        a_c = jnp.cos(ang_a)[None]
        a_s = jnp.sin(ang_a)[None]
        theta16 = theta_of((SQ // 8, LANES))
        k16 = lax.broadcasted_iota(jnp.int32, (SQ // 8, LANES), 0) * 8

        def tables(dev):
            ang_b = (k16 + dev * SQ).astype(f32) * theta16
            b_c = jnp.cos(ang_b)[:, None, :]
            b_s = jnp.sin(ang_b)[:, None, :]
            t_c = (b_c * a_c - b_s * a_s).reshape(SQ, LANES)
            t_s = (b_s * a_c + b_c * a_s).reshape(SQ, LANES)
            return t_c, t_s

        even = (lax.broadcasted_iota(jnp.int32, (SQ, LANES), 1) % 2) == 0

        def rope_half(t, tab):
            cos, sin = tab
            t_next = pltpu.roll(t, LANES - 1, 1)
            t_prev = pltpu.roll(t, 1, 1)
            t_r = jnp.where(even, -t_next, t_prev)
            return t * cos + t_r * sin

        tab_own = tables(my)
        tab_left = tables(left)
        tab_right = tables(right)

        cwk.wait()
        cwv.wait()
        wkv16[:, 0:HD] = wkf[...].astype(bf16)
        wkv16[:, HD:2 * HD] = wvf[...].astype(bf16)

        def project_kv(xb, tab, dst):
            kv = jnp.dot(xb, wkv16[...], preferred_element_type=f32)
            for g in range(2):
                kg = kv[:, g * LANES:(g + 1) * LANES]
                dst[:, g * LANES:(g + 1) * LANES] = rope_half(kg, tab).astype(bf16)
                vg = kv[:, HD + g * LANES:HD + (g + 1) * LANES]
                dst[:, HD + g * LANES:HD + (g + 1) * LANES] = vg.T.astype(bf16)

        project_kv(A[1], tab_own, KVO.at[1])
        s2 = rdma(KVO.at[1], RKV.at[0], right, 4)
        s2.start()
        project_kv(A[0], tab_own, KVO.at[0])
        s3 = rdma(KVO.at[0], RKV.at[1], left, 5)
        s3.start()

        for hf in range(2):
            rows = pl.ds(hf * HALF, HALF)
            rdma(A.at[0, rows], RX.at[0, rows], left, 2 * hf).wait_recv()
        project_kv(RX[0], tab_left, KVC.at[0])
        s4 = rdma(KVC.at[0], RKV.at[2], right, 6)
        s4.start()
        for hf in range(2):
            rows = pl.ds(hf * HALF, HALF)
            rdma(A.at[1, rows], RX.at[1, rows], right, 2 * hf + 1).wait_recv()
        project_kv(RX[1], tab_right, KVC.at[1])
        s5 = rdma(KVC.at[1], RKV.at[3], left, 7)
        s5.start()

        cwq.wait()
        wq16[...] = wqf[...].astype(bf16)
        row_lo = lax.broadcasted_iota(jnp.int32, (LANES, SQ), 0) < DH
        for b in range(B):
            qb = jnp.dot(A[b], wq16[...], preferred_element_type=f32)
            for g in range(2):
                qg = rope_half(qb[:, g * LANES:(g + 1) * LANES], tab_own) * 0.125
                qgt = qg.T
                qt_ref[b * HQ + 2 * g] = jnp.where(row_lo, qgt, 0.0).astype(bf16)
                qt_ref[b * HQ + 2 * g + 1] = jnp.where(row_lo, 0.0, qgt).astype(bf16)

        def attend(jobs, first):
            chains = [(b, kv_ref, h) for (b, kv_ref) in jobs for h in range(HQ)]
            sts = []
            for (b, kv_ref, h) in chains:
                g = h // 2
                kp = kv_ref[:, g * LANES:(g + 1) * LANES]
                sts.append(jnp.dot(kp, qt_ref[b * HQ + h], preferred_element_type=f32))
            pts, ms, ls, alphas = [], [], [], []
            for (b, kv_ref, h), st in zip(chains, sts):
                idx = b * HQ + h
                cmax = jnp.max(st, axis=0, keepdims=True)
                if first:
                    m_new = cmax
                    pt = jnp.exp(st - m_new)
                    l_new = jnp.sum(pt, axis=0, keepdims=True)
                    alpha = None
                else:
                    m_prev = m_ref[idx]
                    m_new = jnp.maximum(m_prev, cmax)
                    alpha = jnp.exp(m_prev - m_new)
                    pt = jnp.exp(st - m_new)
                    l_new = alpha * l_ref[idx] + jnp.sum(pt, axis=0, keepdims=True)
                pts.append(pt.astype(bf16)); ms.append(m_new); ls.append(l_new); alphas.append(alpha)
            accs = []
            for (b, kv_ref, h), pt in zip(chains, pts):
                g, hh = h // 2, h % 2
                vt = kv_ref[hh * DH:(hh + 1) * DH, HD + g * LANES:HD + (g + 1) * LANES]
                accs.append(jnp.dot(vt, pt, preferred_element_type=f32))
            for n, (b, kv_ref, h) in enumerate(chains):
                idx = b * HQ + h
                acc = accs[n] if first else alphas[n] * acc_ref[idx] + accs[n]
                m_ref[idx] = ms[n]
                l_ref[idx] = ls[n]
                acc_ref[idx] = acc

        attend([(0, KVO.at[0])], True)
        attend([(1, KVO.at[1])], True)
        attend([(0, KVC.at[0])], False)
        attend([(1, KVC.at[1])], False)

        cwo.wait()
        wo16[...] = wof[...].astype(bf16)

        rdma(KVO.at[1], RKV.at[0], left, 4).wait_recv()
        attend([(1, RKV.at[0])], False)
        rdma(KVO.at[0], RKV.at[1], right, 5).wait_recv()
        attend([(0, RKV.at[1])], False)

        def finalize_both():
            ctxs = []
            for b in range(B):
                parts = []
                for h in range(HQ):
                    idx = b * HQ + h
                    parts.append(acc_ref[idx] * (1.0 / l_ref[idx]))
                ctx_t = jnp.concatenate(parts, axis=0)
                ctxs.append(ctx_t.T.astype(bf16))
            ctx = jnp.concatenate(ctxs, axis=0)
            o = jnp.dot(ctx, wo16[...], preferred_element_type=f32)
            out_ref[0] = o[0:SQ]
            out_ref[1] = o[SQ:2 * SQ]

        rdma(KVC.at[0], RKV.at[2], left, 6).wait_recv()
        rdma(KVC.at[1], RKV.at[3], right, 7).wait_recv()
        attend([(0, RKV.at[2]), (1, RKV.at[3])], False)
        finalize_both()

        for s in sends + [s2, s3, s4, s5]:
            s.wait_send()

    out = pl.pallas_call(
        body,
        out_shape=jax.ShapeDtypeStruct((B, SQ, D), f32),
        in_specs=[pl.BlockSpec(memory_space=pl.ANY)] * 5,
        out_specs=pl.BlockSpec(memory_space=pltpu.VMEM),
        scratch_shapes=[
            pltpu.VMEM((B, SQ, D), f32),
            pltpu.VMEM((D, HD), f32),
            pltpu.VMEM((D, HD), f32),
            pltpu.VMEM((D, HD), f32),
            pltpu.VMEM((HD, D), f32),
            pltpu.VMEM((B, SQ, D), bf16),
            pltpu.VMEM((2, SQ, D), bf16),
            pltpu.VMEM((2, SQ, 2 * HD), bf16),
            pltpu.VMEM((2, SQ, 2 * HD), bf16),
            pltpu.VMEM((4, SQ, 2 * HD), bf16),
            pltpu.VMEM((D, 2 * HD), bf16),
            pltpu.VMEM((D, HD), bf16),
            pltpu.VMEM((HD, D), bf16),
            pltpu.VMEM((B * HQ, LANES, SQ), bf16),
            pltpu.VMEM((B * HQ, 1, SQ), f32),
            pltpu.VMEM((B * HQ, 1, SQ), f32),
            pltpu.VMEM((B * HQ, DH, SQ), f32),
            pltpu.SemaphoreType.DMA((8,)),
            pltpu.SemaphoreType.DMA((8,)),
            pltpu.SemaphoreType.DMA((8,)),
        ],
        compiler_params=pltpu.CompilerParams(collective_id=0),
    )(x, Wq, Wk, Wv, Wo)
    return out
```

```python
import math

import jax
import jax.numpy as jnp
from jax import lax
from jax.experimental import pallas as pl
from jax.experimental.pallas import tpu as pltpu

N_DEV = 4
B = 2
SQ = 128
D = 512
HQ = 4
DH = 64
HD = HQ * DH
LANES = 128
NPAIR = HQ // 2


def pallas_dist_rope_attn_qseq_b2_sq128_d512_hq4_dh64_kernel(
    x: jax.Array,
    Wq: jax.Array,
    Wk: jax.Array,
    Wv: jax.Array,
    Wo: jax.Array,
):
    bf16 = jnp.bfloat16
    f32 = jnp.float32

    def body(x_hbm, wq_hbm, wk_hbm, wv_hbm, wo_hbm, out_ref,
             xin, wqf, wkf, wvf, wof,
             xb, rx, kv_own, kv_cmp, kv_rcv, wkv16, wq16, wo16,
             qt_ref, m_ref, l_ref, acc_ref,
             lsem, ssem, rsem):
        my = lax.axis_index("i")
        left = (my + N_DEV - 1) % N_DEV
        right = (my + 1) % N_DEV

        bsem = pltpu.get_barrier_semaphore()
        for nb in (left, right):
            pl.semaphore_signal(bsem, inc=1, device_id=(nb,),
                                device_id_type=pl.DeviceIdType.MESH)

        cx = [pltpu.make_async_copy(x_hbm.at[b], xin.at[b], lsem.at[b]) for b in range(B)]
        for c in cx:
            c.start()
        cwk = pltpu.make_async_copy(wk_hbm, wkf, lsem.at[2])
        cwv = pltpu.make_async_copy(wv_hbm, wvf, lsem.at[3])
        cwq = pltpu.make_async_copy(wq_hbm, wqf, lsem.at[4])
        cwo = pltpu.make_async_copy(wo_hbm, wof, lsem.at[5])
        cwk.start()
        cwv.start()

        def rdma(src, dst, dev, i):
            return pltpu.make_async_remote_copy(
                src_ref=src, dst_ref=dst,
                send_sem=ssem.at[i], recv_sem=rsem.at[i],
                device_id=(dev,), device_id_type=pl.DeviceIdType.MESH)

        sends = []
        for b in range(B):
            cx[b].wait()
            xb[b] = xin[b].astype(bf16)
            if b == 0:
                pl.semaphore_wait(bsem, 2)
            s = rdma(xb.at[b], rx.at[b], right if b == 0 else left, b)
            s.start()
            sends.append(s)
        cwq.start()
        cwo.start()

        def theta_of(shape):
            ln = lax.broadcasted_iota(jnp.int32, shape, 1) % DH
            fi = (ln - (ln % 2)).astype(f32)
            return jnp.exp(fi * (-math.log(10000.0) / DH))

        ang_a = lax.broadcasted_iota(jnp.int32, (8, LANES), 0).astype(f32) * theta_of((8, LANES))
        a_c = jnp.cos(ang_a)[None]
        a_s = jnp.sin(ang_a)[None]
        theta16 = theta_of((SQ // 8, LANES))
        k16 = lax.broadcasted_iota(jnp.int32, (SQ // 8, LANES), 0) * 8

        def tables(dev):
            ang_b = (k16 + dev * SQ).astype(f32) * theta16
            b_c = jnp.cos(ang_b)[:, None, :]
            b_s = jnp.sin(ang_b)[:, None, :]
            t_c = (b_c * a_c - b_s * a_s).reshape(SQ, LANES)
            t_s = (b_s * a_c + b_c * a_s).reshape(SQ, LANES)
            return t_c, t_s

        even = (lax.broadcasted_iota(jnp.int32, (SQ, LANES), 1) % 2) == 0

        def rope(t, tab):
            cos, sin = tab
            t_next = pltpu.roll(t, LANES - 1, 1)
            t_prev = pltpu.roll(t, 1, 1)
            return t * cos + jnp.where(even, -t_next, t_prev) * sin

        tab_own = tables(my)
        tab_left = tables(left)
        tab_right = tables(right)

        cwk.wait()
        cwv.wait()
        wkv16[:, 0:HD] = wkf[...].astype(bf16)
        wkv16[:, HD:2 * HD] = wvf[...].astype(bf16)

        def project_kv(xs, tab, dst):
            kv = jnp.dot(xs, wkv16[...], preferred_element_type=f32)
            for g in range(NPAIR):
                dst[2 * g] = rope(kv[:, g * LANES:(g + 1) * LANES], tab).astype(bf16)
                dst[2 * g + 1] = kv[:, HD + g * LANES:HD + (g + 1) * LANES].T.astype(bf16)

        project_kv(xb[1], tab_own, kv_own.at[1])
        s2 = rdma(kv_own.at[1], kv_rcv.at[0], right, 2)
        s2.start()
        project_kv(xb[0], tab_own, kv_own.at[0])
        s3 = rdma(kv_own.at[0], kv_rcv.at[1], left, 3)
        s3.start()

        rdma(xb.at[0], rx.at[0], left, 0).wait_recv()
        project_kv(rx[0], tab_left, kv_cmp.at[0])
        s4 = [rdma(kv_cmp.at[0, p], kv_rcv.at[2, p], right, 4 + 2 * p) for p in range(4)]
        for s in s4:
            s.start()
        rdma(xb.at[1], rx.at[1], right, 1).wait_recv()
        project_kv(rx[1], tab_right, kv_cmp.at[1])
        s5 = [rdma(kv_cmp.at[1, p], kv_rcv.at[3, p], left, 5 + 2 * p) for p in range(4)]
        for s in s5:
            s.start()

        cwq.wait()
        wq16[...] = wqf[...].astype(bf16)
        row_lo = lax.broadcasted_iota(jnp.int32, (LANES, SQ), 0) < DH
        for b in range(B):
            qb = jnp.dot(xb[b], wq16[...], preferred_element_type=f32)
            for g in range(NPAIR):
                qgt = (rope(qb[:, g * LANES:(g + 1) * LANES], tab_own) * 0.125).T
                qt_ref[b * HQ + 2 * g] = jnp.where(row_lo, qgt, 0.0).astype(bf16)
                qt_ref[b * HQ + 2 * g + 1] = jnp.where(row_lo, 0.0, qgt).astype(bf16)

        def scores(jobs, first, pairs):
            chains = [(b, kv, 2 * g + hh) for (b, kv) in jobs for g in pairs for hh in range(2)]
            sts = [jnp.dot(kv[2 * (h // 2)], qt_ref[b * HQ + h], preferred_element_type=f32)
                   for (b, kv, h) in chains]
            pts, ms, ls, alphas = [], [], [], []
            for (b, kv, h), st in zip(chains, sts):
                idx = b * HQ + h
                cmax = jnp.max(st, axis=0, keepdims=True)
                if first:
                    m_new = cmax
                    pt = jnp.exp(st - m_new)
                    l_new = jnp.sum(pt, axis=0, keepdims=True)
                    alpha = None
                else:
                    m_prev = m_ref[idx]
                    m_new = jnp.maximum(m_prev, cmax)
                    alpha = jnp.exp(m_prev - m_new)
                    pt = jnp.exp(st - m_new)
                    l_new = alpha * l_ref[idx] + jnp.sum(pt, axis=0, keepdims=True)
                pts.append(pt.astype(bf16))
                ms.append(m_new)
                ls.append(l_new)
                alphas.append(alpha)
            return chains, pts, ms, ls, alphas

        def pv(state, first):
            chains, pts, ms, ls, alphas = state
            accs = [jnp.dot(kv[2 * (h // 2) + 1, (h % 2) * DH:(h % 2 + 1) * DH, :], pt,
                            preferred_element_type=f32)
                    for (b, kv, h), pt in zip(chains, pts)]
            for n, (b, kv, h) in enumerate(chains):
                idx = b * HQ + h
                acc_ref[idx] = accs[n] if first else alphas[n] * acc_ref[idx] + accs[n]
                m_ref[idx] = ms[n]
                l_ref[idx] = ls[n]

        def attend(jobs, first):
            pv(scores(jobs, first, tuple(range(NPAIR))), first)

        attend([(0, kv_own.at[0])], True)
        attend([(1, kv_own.at[1])], True)
        attend([(0, kv_cmp.at[0])], False)
        attend([(1, kv_cmp.at[1])], False)

        cwo.wait()
        wo16[...] = wof[...].astype(bf16)

        rdma(kv_own.at[1], kv_rcv.at[0], left, 2).wait_recv()
        attend([(1, kv_rcv.at[0])], False)
        rdma(kv_own.at[0], kv_rcv.at[1], right, 3).wait_recv()
        attend([(0, kv_rcv.at[1])], False)

        def outproj(g):
            for b in range(B):
                parts = [acc_ref[b * HQ + 2 * g + hh] * (1.0 / l_ref[b * HQ + 2 * g + hh])
                         for hh in range(2)]
                ctx = jnp.concatenate(parts, axis=0).T.astype(bf16)
                t = jnp.dot(ctx, wo16[g * LANES:(g + 1) * LANES, :], preferred_element_type=f32)
                out_ref[b] = t if g == 0 else out_ref[b] + t

        for g in range(NPAIR):
            for p in (2 * g, 2 * g + 1):
                rdma(kv_cmp.at[0, p], kv_rcv.at[2, p], left, 4 + 2 * p).wait_recv()
                rdma(kv_cmp.at[1, p], kv_rcv.at[3, p], right, 5 + 2 * p).wait_recv()
                if p == 2 * g:
                    st = scores([(0, kv_rcv.at[2]), (1, kv_rcv.at[3])], False, (g,))
            pv(st, False)
            outproj(g)

        for s in sends + [s2, s3] + s4 + s5:
            s.wait_send()

    return pl.pallas_call(
        body,
        out_shape=jax.ShapeDtypeStruct((B, SQ, D), f32),
        in_specs=[pl.BlockSpec(memory_space=pl.ANY)] * 5,
        out_specs=pl.BlockSpec(memory_space=pltpu.VMEM),
        scratch_shapes=[
            pltpu.VMEM((B, SQ, D), f32),
            pltpu.VMEM((D, HD), f32),
            pltpu.VMEM((D, HD), f32),
            pltpu.VMEM((D, HD), f32),
            pltpu.VMEM((HD, D), f32),
            pltpu.VMEM((B, SQ, D), bf16),
            pltpu.VMEM((2, SQ, D), bf16),
            pltpu.VMEM((2, 4, SQ, LANES), bf16),
            pltpu.VMEM((2, 4, SQ, LANES), bf16),
            pltpu.VMEM((4, 4, SQ, LANES), bf16),
            pltpu.VMEM((D, 2 * HD), bf16),
            pltpu.VMEM((D, HD), bf16),
            pltpu.VMEM((HD, D), bf16),
            pltpu.VMEM((B * HQ, LANES, SQ), bf16),
            pltpu.VMEM((B * HQ, 1, SQ), f32),
            pltpu.VMEM((B * HQ, 1, SQ), f32),
            pltpu.VMEM((B * HQ, DH, SQ), f32),
            pltpu.SemaphoreType.DMA((6,)),
            pltpu.SemaphoreType.DMA((12,)),
            pltpu.SemaphoreType.DMA((12,)),
        ],
        compiler_params=pltpu.CompilerParams(collective_id=0),
    )(x, Wq, Wk, Wv, Wo)
```
